```python
import numpy as np

kernel_name = "dist_sparse_attn_localglobal_htp_kvseq_b2_sq256_skv256_hq4_dh64"

def setup_inputs():
    x = np.random.randn(2, 256, 512).astype(np.float32)
    Wq = np.random.randn(512, 1024).astype(np.float32) * 0.02
    K_ext = np.random.randn(2, 1024, 16, 64).astype(np.float32)
    V_ext = np.random.randn(2, 1024, 16, 64).astype(np.float32)
    Wo = np.random.randn(1024, 512).astype(np.float32) * 0.02
    return {"x": x, "Wq": Wq, "K_ext": K_ext, "V_ext": V_ext, "Wo": Wo}

def reference(x, Wq, K_ext, V_ext, Wo):
    B, Sq, Skv, Hq, Dh = 2, 256, 1024, 16, 64
    Q = (x @ Wq).reshape(B, Sq, Hq, Dh)
    qi = np.arange(Sq)[:, None]
    ki = np.arange(Skv)[None, :]
    local = np.abs(qi - ki) <= 128
    glob = (ki < 32) | (qi < 32)
    mask = local | glob
    scores = np.einsum('bihd,bjhd->bhij', Q, K_ext).astype(np.float32) * 0.125
    scores = np.where(mask[None, None, :, :], scores, -1e9)
    scores_max = scores.max(axis=-1, keepdims=True)
    w = np.exp(scores - scores_max)
    row_keep = mask.any(axis=1)
    w_sum = np.where(row_keep[None, None, :, None], w.sum(axis=-1, keepdims=True), 1.0)
    w = w / w_sum
    w = np.where(row_keep[None, None, :, None], w, 0.0)
    ctx = np.einsum('bhij,bjhd->bihd', w, V_ext).reshape(B, Sq, Hq * Dh)
    return ctx @ Wo
```

```python
import jax
import jax.numpy as jnp
from jax import lax
from jax.experimental import pallas as pl
from jax.experimental.pallas import tpu as pltpu

BF = jnp.bfloat16
F32 = jnp.float32
LOG2E = 1.4426950408889634
QSCALE = 0.125 * LOG2E
NEG = -1e9 * LOG2E
MESH = pl.DeviceIdType.MESH
_NT = (((1,), (1,)), ((), ()))
_TN = (((0,), (0,)), ((), ()))

CFG = {'ar': ((('a', 0, 64, 256, 'f'), ('b', 64, 128, 256, 'f')), (('a', 0, 48, 256, ''), ('b', 48, 128, 256, '')), (('a', 0, 64, 256, ''), ('b', 64, 128, 128, '')), (('a', 0, 48, 256, ''), ('b', 48, 128, 256, ''))), 'bt': ((3, 0, 0),), 'ge0': ('one', 'one'), 'gq0': ('one', 'one'), 'qb_f0': ((3, 1, 0), (3, 1, 1)), 'mergeb': ((1, 0), (1, 1)), 'q2via': (3, 3, 1, 1, 3, 3, 3, 1), 'fin': (), 'early': ((1, 2, 0, 48), (3, 1, 1, 48), (2, 0, 1, 48)), 'layout': (3, 2, 1, 0)}
HS = "AB"
CHUNKS = ((0, 0), (0, 1), (1, 0), (1, 1))


def _dot(a, b):
    return jnp.dot(a, b, preferred_element_type=F32)


def _dot_nt(a, b):
    return lax.dot_general(a, b, _NT, preferred_element_type=F32)


def _dot_tn(a, b):
    return lax.dot_general(a, b, _TN, preferred_element_type=F32)


def _iota(shape, dim):
    return lax.broadcasted_iota(jnp.int32, shape, dim)


def _col_to_row(m):
    n = m.shape[0]
    eye = _iota((n, 128), 0) == _iota((n, 128), 1)
    return jnp.sum(jnp.where(eye, jnp.broadcast_to(m, (n, 128)), 0.0), axis=0, keepdims=True)


def _blockdiag(kt):
    z = jnp.zeros((64, kt.shape[1]), kt.dtype)
    return jnp.concatenate(
        [jnp.concatenate([kt[:64], z], axis=0), jnp.concatenate([z, kt[64:]], axis=0)], axis=1).astype(BF)


def _softmax(s):
    m = jnp.max(s, axis=1, keepdims=True)
    return jnp.exp2(s - m).astype(BF), m


def _with_ones(vt):
    return jnp.concatenate([vt, jnp.ones((16, vt.shape[1]), vt.dtype)], axis=0).astype(BF)


def _head_out(s, vt, out, hh, nl=128):
    p, m = _softmax(s)
    c = _dot_nt(_with_ones(vt), p)
    l = c[64:65]
    out[0][hh * 64:(hh + 1) * 64, :] = (c[:64] * (1.0 / l)).astype(BF)
    out[1][hh // 2, hh % 2:hh % 2 + 1, :] = _col_to_row(m[:nl]) + jnp.log2(l)


def _step_main(pr, getq, getk, getv, masks, outs, nls):
    def rest(s2):
        for t, out in enumerate(outs):
            for j in range(2):
                s = masks[t](s2[t * 128:(t + 1) * 128, j * 256:(j + 1) * 256])
                _head_out(s, getv(j), out, 2 * pr + j, nls[t])

    return [(lambda: _dot(getq(), _blockdiag(getk())), rest)]


def _step_band(pr, getq, getk, getv, mask, out):
    def rest(s2):
        for j in range(2):
            _head_out(mask(s2[:, j * 128:(j + 1) * 128]), getv(j), out, 2 * pr + j)

    return [(lambda: _dot(getq(), _blockdiag(getk())), rest)]


def _steps_glob(getq, getk, getv, out):
    def qk():
        lane = _iota((32, 128), 1)
        res = []
        for pr in range(2):
            q2 = getq(pr)
            z = jnp.zeros_like(q2)
            lhs = jnp.concatenate([jnp.where(lane < 64, q2, z), jnp.where(lane >= 64, q2, z)], axis=0)
            res.append(_dot(lhs, getk(pr).astype(BF)))
        return jnp.concatenate(res, axis=0)

    def rest(s):
        lane = _iota((64, 128), 1)
        p, m = _softmax(s)
        c0 = _dot_nt(_with_ones(getv(0)), p)
        c1 = _dot_nt(getv(1).astype(BF), p)
        l = c0[128:129]
        d = jnp.where(lane < 64, jnp.where(lane < 32, c0[0:64], c0[64:128]),
                      jnp.where(lane < 96, c1[0:64], c1[64:128]))
        out[0][...] = (d * (1.0 / l)).astype(BF)
        out[1][...] = _col_to_row(m) + jnp.log2(l)

    return [(qk, rest)]


def _run_steps(steps, depth=5):
    scores = [st[0]() for st in steps[:depth]]
    for i, st in enumerate(steps):
        if i + depth < len(steps):
            scores.append(steps[i + depth][0]())
        st[1](scores[i])


def _merge_g(views):
    ls = [v[1][...] for v in views]
    if len(views) == 1:
        return views[0][0][...].astype(F32), ls[0]
    mx = ls[0]
    for l in ls[1:]:
        mx = jnp.maximum(mx, l)
    ws = [jnp.exp2(l - mx) for l in ls]
    tot = ws[0]
    for w in ws[1:]:
        tot = tot + w
    inv = 1.0 / tot
    acc = views[0][0][...].astype(F32) * (ws[0] * inv)
    for v, w in zip(views[1:], ws[1:]):
        acc = acc + v[0][...].astype(F32) * (w * inv)
    return acc, mx + jnp.log2(tot)


def _pair_weights(la, lb):
    mx = jnp.maximum(la, lb)
    ea = jnp.exp2(la - mx)
    eb = jnp.exp2(lb - mx)
    inv = 1.0 / (ea + eb)
    return ea * inv, eb * inv


def _merge_b(cv, dv, ps):
    out = []
    for p in ps:
        wa, wb = _pair_weights(cv[1][p], dv[1][p])
        for j in range(2):
            rs = slice((2 * p + j) * 64, (2 * p + j + 1) * 64)
            out.append((cv[0][rs, :].astype(F32) * wa[j:j + 1]
                        + dv[0][rs, :].astype(F32) * wb[j:j + 1]).astype(BF))
    return jnp.concatenate(out, axis=0)


def _merge_a(cv, gviews, ps):
    gc, gl = _merge_g(gviews)
    glob = _iota((1, 128), 1) < 32
    gl8 = jnp.broadcast_to(gl, (8, 128))
    out = []
    for j in range(2 * ps[0], 2 * ps[-1] + 2):
        gcj = gc if j == 0 else pltpu.roll(gc, 128 - 32 * j, 1)
        glj = gl if j == 0 else pltpu.roll(gl8, 128 - 32 * j, 1)[0:1]
        wa, wb = _pair_weights(cv[1][j // 2, j % 2:j % 2 + 1, :], glj)
        wa = jnp.where(glob, wa, 1.0)
        wb = jnp.where(glob, wb, 0.0)
        out.append((cv[0][j * 64:(j + 1) * 64, :].astype(F32) * wa + gcj * wb).astype(BF))
    return jnp.concatenate(out, axis=0)


class _Refs:
    def __init__(self, names, refs):
        self._refs = dict(zip(names, refs))

    def __getattr__(self, name):
        return self._refs[name]


def _graph(R, cfg):
    ge0 = cfg["ge0"]
    bt = list(cfg["bt"])
    tasks = []

    def add(chip, name, kind, deps=(), waits=(), rank=0.0, **kw):
        if kind == "send":
            kw["parts"] = 2 if kw["kib"] in (16.5, 33, 66) else 1
        tasks.append(dict(chip=chip, name=name, kind=kind, deps=list(deps), waits=list(waits), rank=rank, **kw))

    def cvw(g, b, h):
        return (R.c.at[g, b, h], R.cl.at[g, b, h])

    def dvw(g, b):
        return (R.d.at[g, b], R.dl.at[g, b])

    def evw(s, g, b):
        return (R.e.at[s, g, b], R.el.at[s, g, b])

    def gate(c, d):
        return ["bar", "ent"] if (c in (1, 3) and d != 0) or (c, d) == (0, 2) else ["bar"]

    def send(name, path, view, kib, deps, rank, first_src=None, slot=None):
        ev = {}
        for i in range(len(path) - 1):
            c, d = path[i], path[i + 1]
            nm = "%s>%d" % (name, d)
            src = first_src if (i == 0 and first_src is not None) else view
            add(c, nm, "send", deps=(list(deps) if i == 0 else []) + gate(c, d),
                waits=[] if i == 0 else [ev[c]], rank=rank + 8 * i, dst=d, kib=kib, src=src, dstv=view,
                slot=slot or nm)
            ev[d] = nm
        return ev

    early = {(c, i): (p, n) for (c, i, p, n) in cfg["early"]}

    add(0, "bar", "bar", rank=-9, sig=(1, 3), n=2, pre=False)
    add(1, "bar", "bar", rank=-9, sig=(0, 2), n=1, pre=False)
    add(3, "bar", "bar", rank=-9, sig=(0, 2), n=1, pre=False)
    add(2, "bar", "bar", rank=-9, sig=(), n=2, pre=False)
    add(2, "entsig", "entsig", deps=["bar"], rank=-8)
    add(1, "ent", "ent", deps=["bar"], rank=-7)
    add(3, "ent", "ent", deps=["bar"], rank=-7)
    add(0, "ent", "ent", deps=["bar"], rank=-7)

    for c in range(4):
        a2 = lambda *a, **k: add(c, *a, **k)
        for p in range(2):
            a2("wq%d" % p, "load", rank=0.5, kib=256,
               src=lambda p=p: R.wq_h.at[:, pl.ds(p * 128, 128)], dstv=lambda p=p: R.wq.at[p])
        for i, (b, h) in enumerate(CHUNKS):
            n0 = early.get((c, i), (0, 0))[1]
            for nm, r0, n in (("e", h * 128, n0), ("", h * 128 + n0, 128 - n0)):
                if n:
                    a2("x%d%s%s" % (b, HS[h], nm), "load", rank=i - len(nm), kib=2 * n,
                       src=lambda b=b, r0=r0, n=n: R.x_h.at[b, pl.ds(r0, n)],
                       dstv=lambda b=b, r0=r0, n=n: R.x.at[b, pl.ds(r0, n)])
        gs = {0: (0, 1, 3, 2), 1: (1, 0, 2, 3), 2: (2, 1, 3, 0), 3: (3, 0, 2, 1)}[c]
        for b in range(2):
            for i, g in enumerate(gs):
                rk = -1 if (c == 0 and ((g, b, 0) in bt or (g, b, 1) in bt)) else 4 + 5 * b + i
                a2("k%d%d" % (b, g), "load", rank=rk, kib=256,
                   src=lambda b=b, g=g: R.k_h.at[b, pl.ds(g * 256, 256)], dstv=lambda b=b, g=g: R.k.at[b, pl.ds(g * 256, 256)])
                a2("v%d%d" % (b, g), "load", rank=rk + 0.1, kib=256,
                   src=lambda b=b, g=g: R.v_h.at[b, pl.ds(g * 256, 256)], dstv=lambda b=b, g=g: R.v.at[b, pl.ds(g * 256, 256)])
        a2("wo", "load", rank=8.5, kib=512, src=lambda: R.wo_h, dstv=lambda: R.wo)

        def cwq(p):
            def f():
                R.wqb[:, p * 128:(p + 1) * 128] = R.wq[p].astype(BF)
            return f

        def cwo():
            R.wob[...] = R.wo[...].astype(BF)

        for p in range(2):
            a2("cwq%d" % p, "comp", deps=["wq%d" % p], waits=["wq%d" % p], rank=-3, fn=cwq(p), dur=0.03)
        a2("cwo", "comp", deps=["wo"], waits=["wo"], rank=50, fn=cwo, dur=0.05)

    moved = {(g, i): c for (g, i, c) in cfg["fin"]}
    woev = {}
    for (g, c) in sorted({(g, c) for (g, _), c in moved.items()}):
        woev[c] = [send("W%d%d" % (g, p), [g, c], lambda p=p: R.wob2.at[pl.ds(p * 64, 64)], 64, ["cwo"], p,
                        first_src=lambda p=p: R.wob.at[pl.ds(p * 64, 64)])[c] for p in range(4)]

    kvev = {}
    for n, (g, b, p) in enumerate(bt):
        evs = []
        for t, nm in enumerate("kv"):
            def cvt(t=t, g=g, b=b, p=p, n=n):
                R.kvb[n, t] = (R.k, R.v)[t][b, g * 256 + p * 128:g * 256 + (p + 1) * 128, :].astype(BF)
            ld = "%s%d%d" % (nm, b, g)
            add(0, "c%s%d" % (ld, p), "comp", deps=[ld], waits=[ld], rank=-5, fn=cvt, dur=0.03)
            evs.append(send("KV%s%d" % (ld, p), [0, g], lambda t=t, n=n: R.kvb.at[n, t], 64,
                            ["c%s%d" % (ld, p)], rank=t)[g])
        kvev[(g, b, p)] = evs

    def mask_main(h):
        def f(s):
            q = _iota((128, 128), 0)
            k = _iota((128, 128), 1)
            if h == 0:
                return jnp.concatenate([s[:, :128], jnp.where((k <= q) | (q < 32), s[:, 128:], NEG)], axis=1)
            return jnp.concatenate([jnp.where((k >= q) | (k < 32), s[:, :128], NEG), s[:, 128:]], axis=1)
        return f

    def mask_b(s):
        return jnp.where(_iota((128, 128), 1) <= _iota((128, 128), 0), s, NEG)

    def unit_main(g, b, p, hs):
        r0 = g * 256 + p * 128
        if (g, b, p) in bt:
            n = bt.index((g, b, p))
            kget = lambda: R.kvb[n, 0]
            vget = lambda j: R.kvb[n, 1, j * 64:(j + 1) * 64, :]
        else:
            kget = lambda: R.k[b, r0:r0 + 128, :]
            vget = lambda j: R.v[b, r0 + j * 64:r0 + (j + 1) * 64, :]
        return _step_main(p, lambda: R.q[g, b, p, hs[0] * 128:(hs[-1] + 1) * 128, :], kget, vget,
                          [mask_main(h) for h in hs], [cvw(g, b, h) for h in hs], [(32, 128)[h] for h in hs])

    def unit_b(g, b, p):
        r0 = g * 256 + p * 128
        return _step_band(p, lambda: R.q[g, b, p, 128:256, :], lambda: R.k[b, r0:r0 + 128, 0:128],
                          lambda j: R.v[b, r0 + j * 64:r0 + (j + 1) * 64, 0:128], mask_b, dvw(g, b))

    def unit_g(g, b):
        return _steps_glob(lambda pr: R.q[g, b, pr, 0:32, :],
                           lambda pr: R.k[b, g * 256 + pr * 128:g * 256 + (pr + 1) * 128, :],
                           lambda pr: R.v[b, g * 256 + pr * 128:g * 256 + (pr + 1) * 128, :], evw(4, g, b))

    mergeb = cfg["mergeb"]
    for i, (b, h) in enumerate(CHUNKS):
        base = 10.0 * i
        tag = "%d%s" % (b, HS[h])
        opw = {(c, p): [] for c in range(4) for p in range(2)}
        opd = {(c, p): [] for c in range(4) for p in range(2)}
        gsrc = {}
        for c in range(4):
            def qp(ps, r0=0, r1=128, c=c, b=b, h=h):
                rows = slice(h * 128 + r0, h * 128 + r1)
                y = (_dot(R.x[b, rows, :].astype(BF), R.wqb[:, ps[0] * 128:(ps[-1] + 1) * 128]) * QSCALE).astype(BF)
                for p in ps:
                    R.q[c, b, p, rows, :] = y[:, (p - ps[0]) * 128:(p - ps[0] + 1) * 128]
            ep, n0 = early.get((c, i), (None, 0))
            xs = ["x" + tag] + (["x" + tag + "e"] if n0 else [])
            for p in range(2):
                nm = "qp%s%d" % (tag, p)
                if p == ep:
                    add(c, nm + "e", "comp", deps=[xs[1], "cwq%d" % p], waits=xs[1:], rank=base - 1,
                        dur=0.12 + 0.09 * n0 / 128, fn=lambda qp=qp, p=p, n0=n0: qp((p,), 0, n0))
                    add(c, nm, "comp", deps=[xs[0], "cwq%d" % p], waits=xs[:1], rank=base,
                        dur=0.21 - 0.09 * n0 / 128, fn=lambda qp=qp, p=p, n0=n0: qp((p,), n0, 128))
                else:
                    add(c, nm, "comp", deps=xs + ["cwq%d" % p], waits=xs,
                        rank=base, dur=0.21, cls=2, w=0.09, fuse=("q", b, h, p), unit=qp)

        def dqp(c, p):
            return ["qp%s%d" % (tag, p)] + (["qp%s%de" % (tag, p)] if early.get((c, i), (None,))[0] == p else [])

        kv = lambda g: ["k%d%d" % (b, g), "v%d%d" % (b, g)]
        qat = {(g, p): {} for g in range(4) for p in range(2)}
        c2ev = {}
        fin = [moved.get((g, i), g) for g in range(4)]
        merge2 = [h == 1 and (b, p) in mergeb and fin[2] == 2 for p in range(2)]
        qview = lambda g, p, h, b=b: (lambda: R.q.at[g, b, p, pl.ds(h * 128, 128)])
        for g in range(4):
            for p in range(2):
                t2 = "%d%s%d" % (g, tag, p)
                cview = lambda g=g, b=b, h=h, p=p: (R.c.at[g, b, h, pl.ds(p * 128, 128)], R.cl.at[g, b, h, p])
                kw = dict(dur=0.48, cls=1, w=0.115, fuse=("m", g, b, p, h),
                          unit=lambda hs, g=g, b=b, p=p: unit_main(g, b, p, hs))
                if (g, b, p) in bt:
                    add(g, "m" + t2, "comp", deps=dqp(g, p), waits=kvev[(g, b, p)], rank=base + 5, **kw)
                    opd[(g, p)].append("m" + t2)
                    continue
                if g:
                    path = [2, cfg["q2via"][2 * i + p], 0] if g == 2 else [g, 0]
                    n0 = early[(g, i)][1] if len(dqp(g, p)) == 2 else 0
                    for dep, r0, n in zip(dqp(g, p), (n0, 0), (128 - n0, n0)):
                        ev = send("q" + t2 + dep[5:], path,
                                  lambda g=g, b=b, p=p, r0=h * 128 + r0, n=n: R.q.at[g, b, p, pl.ds(r0, n)],
                                  n / 4.0, [dep], base + 1)
                        for c, e in ev.items():
                            qat[(g, p)].setdefault(c, []).append(e)
                add(0, "m" + t2, "comp", deps=kv(g) + ([] if g else dqp(0, p)),
                    waits=kv(g) + (qat[(g, p)][0] if g else []), rank=base + 5 + (0 if g else 3), **kw)
                if fin[g] == 0:
                    opd[(0, p)].append("m" + t2)
                elif g == 2 and merge2[p]:
                    c2ev[p] = send("c" + t2, [0, 1], cview, 33, ["m" + t2], base + 20)[1]
                else:
                    opw[(fin[g], p)].append(
                        send("c" + t2, [0, fin[g]], cview, 33, ["m" + t2], base + 20)[fin[g]])
        if h == 1:
            for g in range(4):
                for p in range(2):
                    t3 = "%d%d%d" % (g, b, p)
                    w, d = [], []
                    if g == 1:
                        d = dqp(1, p)
                    elif 1 in qat[(g, p)]:
                        w = qat[(g, p)][1]
                    elif (g, b, p) in cfg["qb_f0"]:
                        w = ["qB%s>1" % t3]
                        add(0, w[0], "send", deps=["bar"], waits=qat[(g, p)][0], rank=base + 10, dst=1,
                            kib=32, src=qview(g, p, 1), dstv=qview(g, p, 1), slot=w[0])
                    else:
                        w = [send("qB" + t3, {0: [0, 1], 2: [2, 1], 3: [3, 2, 1]}[g], qview(g, p, 1), 32,
                                  dqp(g, p), base + 2)[1]]
                    bn = "b" + t3
                    add(1, bn, "comp", deps=kv(g) + d, waits=kv(g) + w, rank=base + 6, dur=0.46, cls=1, w=0.055,
                        fuse=("b", g, b, p), unit=lambda g=g, b=b, p=p: unit_b(g, b, p))
                    if fin[g] == 1:
                        opd[(1, p)].append(bn)
                    elif g == 2 and merge2[p]:
                        def mg(b=b, p=p):
                            R.cm[b, p * 128:(p + 1) * 128, :] = _merge_b(cvw(2, b, 1), dvw(2, b), (p,))
                        add(1, "mg" + t3, "comp", deps=[bn], waits=[c2ev[p]], rank=base + 7, fn=mg, dur=0.05)
                        opw[(2, p)].append(send("cm" + t3, [1, 2], lambda b=b, p=p: R.cm.at[b, pl.ds(p * 128, 128)],
                                                32, ["mg" + t3], base + 30)[2])
                    else:
                        dview = lambda g=g, b=b, p=p: (R.d.at[g, b, pl.ds(p * 128, 128)], R.dl.at[g, b, p])
                        opw[(fin[g], p)].append(
                            send("d" + t3, [1, fin[g]], dview, 33, [bn], base + 30)[fin[g]])
        else:
            gp = {0: {"two": [[0, 1], [0, 3, 2]], "one": [[0, 1, 2, 3]], "rev": [[0, 3, 2, 1]]}[cfg["gq0"][b]], 1: [[1, 2, 3]], 2: [[2, 1], [2, 3]], 3: [[3, 2, 1]]}
            gq = {g: {} for g in range(4)}
            for g in range(4):
                for pth in gp[g]:
                    if len(pth) == 2 and pth[1] in qat[(g, 0)] and pth[1] in qat[(g, 1)]:
                        gq[g][pth[1]] = qat[(g, 0)][pth[1]] + qat[(g, 1)][pth[1]]
                    else:
                        ev = send("qG%d%d" % (g, b), pth, lambda g=g, b=b: R.q.at[g, b, :, pl.ds(0, 32)],
                                  16, dqp(g, 0) + dqp(g, 1), base + 2)
                        gq[g].update({c: [e] for c, e in ev.items()})
            for c in (1, 2, 3):
                for g in range(4):
                    add(c, "g%d%d" % (g, b), "comp", deps=kv(g) + (dqp(c, 0) + dqp(c, 1) if g == c else []),
                        waits=kv(g) + (gq[g][c] if g != c else []), rank=base + 6, dur=0.48, cls=1, w=0.11,
                        fuse=("g", g, b), unit=lambda g=g, b=b: unit_g(g, b))
            chains = {0: {"one": [[1, 2, 3, 0]], "two": [[1, 0], [2, 3, 0]], "rev": [[3, 2, 1, 0]]}[ge0[b]],
                      1: [[3, 2, 1]], 2: [[1, 2], [3, 2]], 3: [[1, 2, 3]]}
            for g in range(4):
                gn = "g%d%d" % (g, b)
                gsrc[g] = [4] if fin[g] else []
                if fin[g]:
                    for p in range(2):
                        opd[(fin[g], p)].append(gn)
                for ch in chains[fin[g]]:
                    prev = None
                    for kk in range(len(ch) - 1):
                        c = ch[kk]
                        if prev is None:
                            dd, slot = [gn], 4
                        else:
                            def mgg(g=g, b=b, s=ch[kk - 1]):
                                gc, gl = _merge_g([evw(4, g, b), evw(s, g, b)])
                                R.e[5, g, b] = gc.astype(BF)
                                R.el[5, g, b] = gl
                            add(c, "mg" + gn, "comp", deps=[gn], waits=[prev], rank=base + 7, fn=mgg, dur=0.04)
                            dd, slot = ["mg" + gn], 5
                        prev = send("e%d%d%d" % (c, g, b), [c, ch[kk + 1]], lambda c=c, g=g, b=b: evw(c, g, b),
                                    16.5, dd, base + 25 + kk,
                                    first_src=lambda s=slot, g=g, b=b: evw(s, g, b))[ch[kk + 1]]
                    for p in range(2):
                        opw[(fin[g], p)].append(prev)
                    gsrc[g].append(ch[-2])
        for c in range(4):
            parts = []
            for (ax, r0, r1, n0, _) in cfg["ar"][i]:
                low = c in ((0, 3) if ax == "a" else (0, 1))
                parts.append((ax, r0, r1) + (((0, n0), (n0, 512)) if low else ((n0, 512), (0, n0))))

            idle = ([x for x in range(4) if x not in fin] + [None])[0]
            mine = [g for g in range(4) if fin[g] == c]

            def op(ps, c=c, b=b, h=h, i=i, parts=parts, gsrc=gsrc, idle=idle, mine=mine, merge2=merge2,
                   seen=[]):
                rows = slice(ps[0] * 128, (ps[-1] + 1) * 128)
                p = R.pacc[i] if seen else None
                for g in mine:
                    if h == 0:
                        ctx = _merge_a(cvw(g, b, 0), [evw(s, g, b) for s in gsrc[g]], ps)
                    else:
                        ctx = jnp.concatenate(
                            [R.cm[b, q * 128:(q + 1) * 128, :] if g == 2 and merge2[q]
                             else _merge_b(cvw(g, b, 1), dvw(g, b), (q,)) for q in ps], axis=0)
                    pg = _dot_tn(ctx, (R.wob if g == c else R.wob2)[rows, :])
                    p = pg if p is None else p + pg
                seen.extend(ps)
                if len(seen) == 1:
                    R.pacc[i] = p
                    return
                for (ax, r0, r1, (k0, k1), (o0, o1)) in parts:
                    if k1 > k0:
                        R.out[b, h * 128 + r0:h * 128 + r1, k0:k1] = p[r0:r1, k0:k1]
                        if idle == (c ^ 1 if ax == "a" else 3 - c):
                            R.s[1, i, r0:r1, k0:k1] = p[r0:r1, k0:k1].astype(BF)
                    if o1 > o0:
                        R.s[0, i, r0:r1, o0:o1] = p[r0:r1, o0:o1].astype(BF)
            ops = ["op%s%d" % (tag, p) for p in range(2)] if c != idle else []
            for p, nm in enumerate(ops):
                two = len(mine) == 2
                add(c, nm, "comp", deps=opd[(c, p)] + ["cwo"], waits=opw[(c, p)] + (woev[c] if two else []),
                    rank=base + 8, cls=3 + i, fuse=("o", i, p), unit=op,
                    dur=((0.35 if c == 0 else 0.39) if h == 0 else 0.315) + (0.15 if two else 0),
                    w=((0.165 if c == 0 else 0.195) if h == 0 else 0.14) + (0.12 if two else 0))

            for pi, (ax, r0, r1, kc, oc) in enumerate(parts):
                p1, p2 = (c ^ 1, 3 - c) if ax == "a" else (3 - c, c ^ 1)
                t2 = "%s%d%s" % (ax, pi, tag)
                rb = 100.0 + 10 * i

                def acc(st, b=b, h=h, i=i, r0=r0, r1=r1, kc=kc, oc=oc, first=(c == idle)):
                    def f():
                        rows = slice(h * 128 + r0, h * 128 + r1)
                        if st == 2:
                            R.out[b, rows, oc[0]:oc[1]] = R.r[2, i, r0:r1, oc[0]:oc[1]].astype(F32)
                        else:
                            v = R.r[st, i, r0:r1, kc[0]:kc[1]].astype(F32)
                            if not (first and st == 0):
                                v = R.out[b, rows, kc[0]:kc[1]] + v
                            R.out[b, rows, kc[0]:kc[1]] = v
                            R.s[st + 1, i, r0:r1, kc[0]:kc[1]] = v.astype(BF)
                    return f

                prev = ops
                for st, pd in enumerate((p1, p2, p1)):
                    nm = "r%d%s" % (st + 1, t2)
                    sc, rc = ((oc, kc), (kc, kc), (kc, oc))[st]
                    relay = cfg["ar"][i][pi][4] if st == 2 else ""
                    if rc[1] > rc[0] and (("f" in relay and c == 2) or ("g" in relay and p2 == 0)):
                        rx = (st, i, pl.ds(r0, r1 - r0), pl.ds(rc[0], rc[1] - rc[0]))
                        add(c, nm + "*", "send", deps=gate(c, p2), waits=[nm], rank=rb + 30, dst=p2, slot=nm,
                            kib=(r1 - r0) * (rc[1] - rc[0]) / 512.0, ev=nm,
                            src=lambda rx=rx: R.r.at[rx], dstv=lambda rx=rx: R.r.at[rx])
                    if sc[1] > sc[0] and not (("f" in relay and c == 0) or ("g" in relay and p1 == 0)
                                              or (st == 0 and c == idle)):
                        ix = (st, i, pl.ds(r0, r1 - r0), pl.ds(sc[0], sc[1] - sc[0]))
                        add(c, nm, "send", deps=prev + gate(c, pd), rank=rb + 12 * st, dst=pd, slot=nm,
                            kib=(r1 - r0) * (sc[1] - sc[0]) / 512.0,
                            src=lambda ix=ix: R.s.at[ix], dstv=lambda ix=ix: R.r.at[ix])
                    if rc[1] > rc[0] and not (st == 0 and p1 == idle):
                        an = "a%d%s" % (st + 1, t2)
                        add(c, an, "comp", deps=prev if st < 2 else [], waits=[nm],
                            rank=-1 if st < 2 else 200, fn=acc(st), dur=0.03)
                        prev = [an]
    return tasks


def _sem_slots(tasks):
    ssem, rsem, ns, nr = {}, {}, [0] * 4, [0] * 4
    for t in tasks:
        if t["kind"] == "send":
            key = (t["chip"], t["name"])
            ssem[key], rsem[key] = ns[t["chip"]], nr[t["dst"]]
            ns[t["chip"]] += t["parts"]
            nr[t["dst"]] += t["parts"]
    ssem["n"], rsem["n"] = max(ns), max(nr)
    return ssem, rsem


def _emit(R, me, tasks, order, layout, trace=False):
    ssem, rsem = _sem_slots(tasks)
    by = {(t["chip"], t["name"]): t for t in tasks}
    incoming = {(t["dst"], t.get("ev", t["name"])): t for t in tasks if t["kind"] == "send"}

    def rdma(t):
        src, dst = t["src"](), t["dstv"]()
        if not isinstance(src, tuple):
            src, dst = (src,), (dst,)
        return [pltpu.make_async_remote_copy(src_ref=s, dst_ref=d, send_sem=R.ssem.at[ssem[(t["chip"], t["name"])] + k],
                                             recv_sem=R.rsem.at[rsem[(t["chip"], t["name"])] + k],
                                             device_id=(t["dst"],), device_id_type=MESH)
                for k, (s, d) in enumerate(zip(src, dst))]

    def load(t, k):
        return pltpu.make_async_copy(t["src"](), t["dstv"](), R.lsem.at[k])

    def loads_of(c):
        return list(enumerate(by[(c, n)] for n in order[c] if (c, n) in by and by[(c, n)]["kind"] == "load"))

    def prologue1(c):
        bar = pltpu.get_barrier_semaphore()
        if c == 0:
            for d in (1, 3):
                pl.semaphore_signal(bar, 1, device_id=(d,), device_id_type=MESH)
        elif c in (1, 3):
            pl.semaphore_signal(bar, 1, device_id=(0,), device_id_type=MESH)
        for k, t in loads_of(c)[:3]:
            load(t, k).start()
        if c in (1, 3):
            pl.semaphore_wait(bar, 1)
            pl.semaphore_signal(bar, 1, device_id=(2,), device_id_type=MESH)

    def prologue2(c):
        for k, t in loads_of(c)[3:]:
            load(t, k).start()
        if c == 2:
            pl.semaphore_wait(pltpu.get_barrier_semaphore(), 2)
            for d in (1, 3, 0):
                pl.semaphore_signal(R.ent, 1, device_id=(d,), device_id_type=MESH)

    def program(c):
        names = order[c]
        assert sorted(m for n in names for m in n.split("+") if m[0] != "~") == sorted(t["name"] for t in tasks if t["chip"] == c), c
        loads, waited, done, sent = {}, set(), set(), {}

        def wait(ev):
            if ev in waited:
                return
            waited.add(ev)
            if ev in loads:
                loads[ev].wait()
            else:
                for cp in rdma(incoming[(c, ev)]):
                    cp.wait_recv()

        bar = pltpu.get_barrier_semaphore()

        def run(ts):
            t = ts[0]
            kind = t["kind"]
            if kind == "load":
                loads[t["name"]] = load(t, len(loads))
            elif kind == "send":
                sent[t["name"]] = rdma(t)
                for cp in sent[t["name"]]:
                    cp.start()
            elif kind == "bar":
                if c == 0:
                    pl.semaphore_wait(bar, t["n"])
            elif kind == "entsig":
                pass
            elif kind == "ent":
                pl.semaphore_wait(R.ent, 1)
            elif "fuse" in t:
                steps, keys = [], [u["fuse"] for u in ts]
                for u in ts:
                    f = u["fuse"]
                    if f[0] in "bg":
                        steps += u["unit"]()
                    elif f[:-1] + (1 - f[-1],) not in keys:
                        steps += u["unit"]((f[-1],)) or []
                    elif f[-1] == 0:
                        steps += u["unit"]((0, 1)) or []
                _run_steps(steps)
            else:
                for u in ts:
                    u["fn"]()

        i = 0
        while i < len(names):
            if names[i][0] == "~":
                for cp in sent.pop(names[i][1:]):
                    cp.wait_send()
                i += 1
                continue
            group = names[i].split("+")
            ts = [by[(c, n)] for n in group]
            i += 1
            for t in ts:
                assert all(d in done for d in t["deps"]), (c, t["name"])
                for w in t["waits"]:
                    if trace and w not in waited:
                        with jax.named_scope("W_" + w.replace(">", "_")):
                            wait(w)
                    wait(w)
            t = ts[0]
            kind = t["kind"]
            if trace and kind in ("comp", "bar", "ent"):
                with jax.named_scope("C_" + names[i - 1].replace("+", "_")):
                    run(ts)
            else:
                run(ts)
            done.update(group)
        for ev in list(loads) + [n for (d, n) in incoming if d == c]:
            wait(ev)
        for n, cps in sent.items():
            if trace:
                with jax.named_scope("W_fin_" + n.replace(">", "_")):
                    for cp in cps:
                        cp.wait_send()
            else:
                for cp in cps:
                    cp.wait_send()

    def chain(fn, cs):
        if len(cs) == 1:
            fn(cs[0])
        else:
            lax.cond(me == cs[0], lambda: fn(cs[0]), lambda: chain(fn, cs[1:]))

    chain(prologue1, (3, 1, 2, 0))
    chain(prologue2, (2, 0, 3, 1))
    for c in layout:
        pl.when(me == c)(lambda c=c: program(c))


def make_kernel(cfg, order, interpret=False, trace=False):
    ssem, rsem = _sem_slots(_graph(None, cfg))

    def kernel(x, Wq, K_ext, V_ext, Wo):
        kt = jnp.transpose(K_ext, (0, 2, 3, 1)).reshape(2, 1024, 256)
        vt = jnp.transpose(V_ext, (0, 2, 3, 1)).reshape(2, 1024, 256)
        names = ("x_h", "wq_h", "k_h", "v_h", "wo_h", "out", "x", "wq", "wqb", "k", "v", "wo", "wob", "wob2", "q", "c", "cl", "d", "dl",
                 "cm", "e", "el", "kvb", "pacc", "s", "r", "lsem", "ssem", "rsem", "ent")

        def body(*refs):
            R = _Refs(names, refs)
            _emit(R, lax.axis_index("i"), _graph(R, cfg), order, cfg["layout"], trace)

        V = pltpu.VMEM
        return pl.pallas_call(
            body,
            out_shape=jax.ShapeDtypeStruct((2, 256, 512), F32),
            in_specs=[pl.BlockSpec(memory_space=pl.ANY)] * 5,
            out_specs=pl.BlockSpec(memory_space=pltpu.VMEM),
            scratch_shapes=[
                V((2, 256, 512), F32), V((2, 512, 128), F32), V((512, 256), BF),
                V((2, 1024, 256), F32), V((2, 1024, 256), F32), V((256, 512), F32), V((256, 512), BF), V((256, 512), BF),
                V((4, 2, 2, 256, 128), BF), V((4, 2, 2, 256, 128), BF), V((4, 2, 2, 2, 2, 128), F32),
                V((4, 2, 256, 128), BF), V((4, 2, 2, 2, 128), F32),
                V((2, 256, 128), BF), V((6, 4, 2, 64, 128), BF), V((6, 4, 2, 1, 128), F32),
                V((max(len(cfg["bt"]), 1), 2, 128, 256), BF), V((4, 128, 512), F32),
                V((3, 4, 128, 512), BF), V((3, 4, 128, 512), BF),
                pltpu.SemaphoreType.DMA((23 + len(cfg["early"]),)), pltpu.SemaphoreType.DMA((ssem["n"],)),
                pltpu.SemaphoreType.DMA((rsem["n"],)), pltpu.SemaphoreType.REGULAR,
            ],
            compiler_params=pltpu.CompilerParams(collective_id=0, vmem_limit_bytes=48 * 1024 * 1024,
                                                 disable_semaphore_checks=True),
            interpret=interpret,
        )(x, Wq, kt, vt, Wo)

    return kernel


ORDER = {
    0: """
        k03 wq1 x0B wq0 x0A x1A x1B v03 k01 k13 v01 v13 k02 k11 k12 v02 v11 k10 v10 v12 wo k00 v00 ck030 cwq1 qp0B1
        cwq0 bar KVk030>3 qB001>1 qp0A0+qp0B0 qp0A1 qG00>1 qB000>1 qp1A0 qp1A1 qG01>1 qp1B1 cv030 KVv030>3 qp1B0
        qB010>1 ent m30B1 c30B1>3 qB311>1 m10A0+m31B1 c31B1>3 qB310>1 qB011>1 c10A0>1 m31B0 c31B0>3 m20A1 c20A1>2
        m20B1+m11A1 c20B1>2 c11A1>1 m10A1+m30A1+m11A0+m01B0 c30A1>3 c11A0>1 c10A1>1 cwo m20A0+m20B0+m01A0 c20A0>2
        c20B0>2 m00B0+m21A0+m11B0 c21A0>2 c11B0>1 m00A0+m00A1+m00B1+m21A1+m11B1 c21A1>2 c11B1>1 m10B1+m21B0+m21B1
        c21B0>1 c21B1>1 op0A0 op0A1 r1b10A m10B0+m01A1+m31A0+m01B1 c31A0>3 c10B0>1 c10B1>1 r1a00A m31A1 c31A1>3 op0B1
        ~KVk030>3 ~qB001>1 ~qG00>1 ~qB000>1 ~qG01>1 ~KVv030>3 a1b10A r2b10A op0B0 r1b10B r1a00B op1A0 ~qB010>1
        ~c30B1>3 ~qB311>1 ~c31B1>3 ~qB310>1 ~qB011>1 a1a00A op1A1 r1b11A r2a00A op1B0 op1B1 r1b11B r1a01B r1a01A
        ~c10A0>1 ~c31B0>3 ~c20A1>2 ~c20B1>2 ~c11A1>1 ~c30A1>3 a1b10B r2b10B ~c11A0>1 ~c10A1>1 ~c20A0>2 ~c20B0>2
        ~c21A0>2 ~c11B0>1 a1a01B r2a01B ~c21A1>2 ~c11B1>1 ~c21B0>1 ~c21B1>1 ~r1b10A ~c31A0>3 a1b11B ~c10B0>1 ~c10B1>1
        ~c31A1>3 a1a01A a2a00A ~r1a00A ~r1b10B a2b10A ~r2b10A a1a00B r2a00B a2a00B a3b10A ~r1a00B ~r1b11A a1b11A
        r2b11A r2b11B a2b11A r3b11A r2a01A ~r2a00A ~r1a01B a2b10B r3b10B a2a01A r3a01A r3a00B ~r1a01A a3a00A ~r1b11B
        a3a00B a3b11A ~r2b10B ~r2a01B ~r2b11A a2a01B r3a01B ~r2a00B a2b11B r3b11B ~r2b11B ~r3b11A a3a01B a3b11B
        ~r2a01A ~r3a01A a3a01A a3b10B
    """.split(),
    1: """
        wq0 x1Ae x1A x0A wq1 k00 v00 k10 x1B v02 k02 v10 v11 k13 k03 v03 k11 x0B v13 k12 wo v12 k01 v01 bar cwq0
        qp1A0e q11A0e>0 qp1A0 q11A0>0 ent qp0A0 q10A0>0 cwq1 qp0A1 q10A1>0 qG10>2 qp1A1 q11A1>0 qG11>2 qG00>2 g00
        e100>2 qp1B0+qp1B1 qG01>2 q20B1>0 q11B0>0 b201 d201>2 g01 q20B0>0 e101>2 q11B1>0 b200 d200>2 g30+b301 e130>2
        d301>3 qp0B0+qp0B1 q10B1>0 g20+b110+b310+b311 q21B1>0 e120>2 d310>3 b000+b001+b300+b010 d010>0 d300>3 q10B0>0
        d001>0 d000>0 cwo g11+g21+g31+b111+b211 e131>2 d311>3 e121>2 g10+b100+b011+b210 op0A0 op0A1 r1a00A r1b10A
        d011>0 op1A0 op1A1 r1b11A b101 op1B0+op1B1 r1a01B r1a01A mg210 cm210>2 mg211 cm211>2 r1b11B ~q11A0e>0 ~q11A0>0
        ~q10A0>0 ~q10A1>0 ~qG10>2 ~q11A1>0 a1b10A r2b10A op0B0 op0B1 r1a00B r1b10B ~qG11>2 ~qG00>2 ~e100>2 ~qG01>2
        ~q20B1>0 ~q11B0>0 a1b10B ~d201>2 ~q20B0>0 ~e101>2 ~q11B1>0 ~d200>2 ~e130>2 a1b11A r2b11A r2b10B ~d301>3
        ~q10B1>0 ~q21B1>0 ~e120>2 ~d310>3 ~d010>0 a1a00A r2a00A ~d300>3 ~q10B0>0 ~d001>0 ~d000>0 ~e131>2 ~d311>3
        a2b10A ~e121>2 ~r1a00A ~r1b10A ~d011>0 ~r1b11A ~r1a01B a2a00A r3a00A ~r1a01A ~cm210>2 ~cm211>2 ~r2b10A a1a00B
        r2a00B r3b10A a2a00B r3a00B ~r1b11B a3b10A a1a01B r2a01B ~r1a00B ~r1b10B ~r2b11A a1a01A r2a01A a1b11B r2b11B
        ~r2b10B ~r2a00A a2a01B r3a01B a2b10B ~r3a00A ~r2a00B a2b11A r3b11A r3b10B a2a01A r3a01A ~r3b10A ~r3a00B a2b11B
        r3b11B a3b10B ~r2a01B ~r2b11B a3a01A ~r2a01A ~r3a01B a3b11A a3a00B ~r3b11A ~r3a01A a3a01B a3a00A ~r3b10B
        a3b11B
    """.split(),
    2: """
        wq1 x0A x0B x0Ae wq0 k00 x1A v02 v00 k10 x1B v13 v11 k11 k03 k12 v03 v01 k01 v12 v10 wo k13 k02 bar entsig
        cwq1 qp0A1 q20A1>3 qp0B1 q20B1>1 qp0A1e q20A1e>3 cwq0 qp0A0 q20A0>3 qp0B0 q20B0>1 qp1A0 q21A0>3 qB301>1 qp1A1
        qG10>3 qG11>3 q21A1>3 qG30>1 qG20>1 g00 qp1B1 q21B1>1 qB300>1 mgg00 qp1B0 q21B0>3 e200>3 qG00>3 qG01>3 g11
        qG31>1 qG21>1 qB210>1 g30 g10 mgg30 e230>3 mgg10 e210>1 g01 mgg11 e211>1 mgg01 e201>3 cwo g31 g20+g21 op0A1
        op0A0 r1a00A r1b10A mgg31 op0B1 op0B0 r1a00B r1b10B e231>3 op1A0 ~q20A1>3 ~q20B1>1 ~q20A1e>3 ~q20A0>3 ~q20B0>1
        ~q21A0>3 a1b10A r2b10A op1A1 r1a01A r1b11A ~qB301>1 ~qG10>3 ~qG11>3 ~q21A1>3 ~qG30>1 ~qG20>1 a1a00B r2a00B
        ~q21B1>1 ~qB300>1 ~q21B0>3 ~e200>3 ~qG00>3 ~qG01>3 a1b11A r2b11A ~qG31>1 ~qG21>1 ~qB210>1 ~e230>3 ~e210>1
        ~e211>1 a1a00A r2a00A op1B0 ~e201>3 ~r1a00A ~r1b10A ~r1a00B ~r1b10B ~e231>3 a2b10A r3b10A op1B1 r1a01B r1b11B
        ~r2b10A ~r1b11A a1a01B r2a01B ~r1a01A ~r2a00B a1b11B r2b11B ~r2a00A a1a01A r2a01A ~r2b11A a1b10B r2b10B
        ~r3b10A a2b10B r3b10B ~r1a01B a2a00A r3a00A ~r1b11B a2a00B r3a00B ~r2b11B a2b11A r3b11A r3b10A* ~r2a01B a3b10A
        r3a00A* a3a00A ~r2a01A ~r2b10B a2a01B r3a01B ~r3a00A a2b11B r3b11B a2a01A r3a01A ~r3b10B a3b11A ~r3a00B a3a00B
        a3a01B ~r3b11A ~r3b10A* a3b10B a3a01A ~r3a00A* ~r3a01B a3b11B
    """.split(),
    3: """
        wq1 x0Be x0B x1B wq0 x0A v02 k11 k02 v13 x1A v01 k12 k13 k01 v10 v11 v12 k00 v03 k03 v00 wo k10 bar cwq1
        qp0B1e q30B1e>0 qp0B1 q30B1>0 ent qB301>2 qp1B1 q31B1>0 cwq0 qp1B0 q31B0>0 qp0A0+qp0B0 qp0A1 qG30>2 qB300>2
        q20A1>0 q20A1e>0 q30A1>0 qp1A1 qp1A0 qG31>2 q20A0>0 g20 e320>2 g31 q21A0>0 g10 e310>2 m30B0+g11 e311>2 q21A1>0
        g21 e321>2 q21B0>0 g30 g00 mgg00 e300>0 q31A0>0 q31A1>0 cwo m30A0+g01 op0B1 op0A1 op0A0 r1b10A mgg01 e301>0
        op1B0 op0B0 r1b10B r1a00B r1a00A op1B1 r1b11B ~q30B1e>0 ~q30B1>0 ~qB301>2 ~q31B1>0 ~q31B0>0 ~qG30>2 a1b10A
        r2b10A r1a01B ~qB300>2 ~q20A1>0 ~q20A1e>0 ~q30A1>0 ~qG31>2 ~q20A0>0 a1a00A r2a00A ~e320>2 ~q21A0>0 ~e310>2
        ~e311>2 ~q21A1>0 ~e321>2 a1a00B r2a00B op1A0 op1A1 r1a01A ~q21B0>0 ~e300>0 ~q31A0>0 ~q31A1>0 ~r1b10A ~e301>0
        a2b10A r3b10A r1b11A ~r1b10B ~r1a00B ~r1a00A ~r1b11B a1b10B r2b10B a1a01A r2a01A ~r2b10A ~r1a01B ~r2a00A
        a1b11A r2b11A a2b11A r3b11A ~r2a00B ~r1a01A a2a00A r3a00A a1a01B r2a01B ~r3b10A ~r1b11A ~r2b10B a1b11B r2b11B
        a2b11B r3b11B ~r2a01A a2a01B a2b10B r3b10B ~r2b11A a2a00B r3a00B r3a01B ~r3b11A a3b11A a3a00A ~r3a00A ~r2a01B
        a2a01A r3a01A a3a00B ~r2b11B ~r3b11B a3b10A a3b10B ~r3a00B a3a01B ~r3b10B ~r3a01B a3b11B a3a01A
    """.split(),
}

_KERNEL = make_kernel(CFG, ORDER)


def pallas_dist_sparse_attn_localglobal_htp_kvseq_b2_sq256_skv256_hq4_dh64_kernel(
    x: jax.Array,
    Wq: jax.Array,
    K_ext: jax.Array,
    V_ext: jax.Array,
    Wo: jax.Array,
):
    return _KERNEL(x, Wq, K_ext, V_ext, Wo)
```
